```python
import numpy as np

kernel_name = "dist_sort_i_m128_n64"

def setup_inputs():
    return {"x": np.random.randn(512, 64).astype(np.float32)}

def reference(x: np.ndarray) -> np.ndarray:
    return np.sort(x, axis=0)
```

```python
import jax
import jax.numpy as jnp
from jax import lax
from jax.experimental import pallas as pl
from jax.experimental.pallas import tpu as pltpu

_MESH = pl.DeviceIdType.MESH
_F32 = jnp.float32
_mn, _mx, _sel = jnp.minimum, jnp.maximum, jnp.where

_NET16 = (
    (0, 13), (1, 12), (2, 15), (3, 14), (4, 8), (5, 6), (7, 11), (9, 10),
    (0, 5), (1, 7), (2, 9), (3, 4), (6, 13), (8, 14), (10, 15), (11, 12),
    (0, 1), (2, 3), (4, 5), (6, 8), (7, 9), (10, 11), (12, 13), (14, 15),
    (0, 2), (1, 3), (4, 10), (5, 11), (6, 7), (8, 9), (12, 14), (13, 15),
    (1, 2), (3, 12), (4, 6), (5, 7), (8, 10), (9, 11), (13, 14),
    (1, 4), (2, 6), (5, 8), (7, 10), (9, 13), (11, 14),
    (2, 4), (3, 6), (9, 12), (11, 13),
    (3, 5), (6, 8), (7, 9), (10, 12),
    (3, 4), (5, 6), (7, 8), (9, 10), (11, 12),
    (6, 7), (8, 9),
)


def _iotas():
    return (lax.broadcasted_iota(jnp.int32, (8, 128), 0),
            lax.broadcasted_iota(jnp.int32, (8, 128), 1))


def _sperm(v, idx):
    return jnp.take_along_axis(v, idx, axis=0, mode="promise_in_bounds")


def _sxor(v, d):
    if d == 4:
        return pltpu.roll(v, 4, 0)
    return _sperm(v, _iotas()[0] ^ d)


def _skew_roll(v, shift):
    return pltpu.roll(v, shift, 1, stride=2, stride_axis=0)


def _pack(lo, hi):
    return pltpu.pack_elementwise([lo, hi], packed_dtype=jnp.bfloat16)


def _unpack(p, index):
    return pltpu.unpack_elementwise(
        p, index=index, packed_dtype=jnp.bfloat16, unpacked_dtype=_F32)


def _oe_merge(a, b, first, second):
    if len(a) == 1:
        return [first(a[0], b[0]), second(a[0], b[0])]
    even = _oe_merge(a[0::2], b[0::2], first, second)
    odd = _oe_merge(a[1::2], b[1::2], first, second)
    out = [even[0]]
    for p, q in zip(odd[:-1], even[1:]):
        out += [first(p, q), second(p, q)]
    return out + [odd[-1]]


def _swap_stage(v, d, first, second):
    mask = (_iotas()[0] & d) != 0
    out = []
    for a, b in zip(v[0::2], v[1::2]):
        p = _sel(mask, b, a)
        q = _sxor(_sel(mask, a, b), d)
        out += [first(p, q), second(p, q)]
    return out


def _bitonic32(v, first, second):
    v = [first(v[0], v[2]), first(v[1], v[3]), second(v[0], v[2]), second(v[1], v[3])]
    v = [first(v[0], v[1]), second(v[0], v[1]), first(v[2], v[3]), second(v[2], v[3])]
    for d in (4, 2, 1):
        v = _swap_stage(v, d, first, second)
    return v


def _spread(x):
    sub, lane = _iotas()
    q = {}
    for w0 in range(2):
        h = ((lane + w0) >> 1) + sub
        odd = ((lane ^ w0) & 1) == 1
        t = [_sperm(_sel(odd, x[2 * j + 1], x[2 * j]), h & 7) for j in range(2)]
        hi = (h & 8) != 0
        q[0, w0] = _sel(hi, t[1], t[0])
        q[1, w0] = _sel(hi, t[0], t[1])
    return [_skew_roll(q[w1, w0], 32 * k + 16 * w1 + w0)
            for w0 in range(2) for w1 in range(2) for k in range(4)]


def _sort_half(src_ref, row0, dst_ref):
    _, lane = _iotas()
    f, s = _mx, _mn
    r = _spread([src_ref[pl.ds(row0 + 8 * t, 8), :] for t in range(4)])
    v = [None] * 16
    for n, (i, j) in enumerate(_NET16[:8]):
        v[i], v[j] = r[2 * n], r[2 * n + 1]
    for i, j in _NET16:
        v[i], v[j] = f(v[i], v[j]), s(v[i], v[j])
    v = _oe_merge(v[0::2], [_sxor(t, 4) for t in v[1::2]], f, s)
    v = _swap_stage(v, 4, f, s)
    v = _oe_merge(v[0::2], [_sxor(t, 6) for t in v[1::2]], f, s)
    v = _swap_stage(v, 4, f, s)
    v = _swap_stage(v, 2, f, s)
    a, b = v[0::2], [_sxor(t, 7) for t in v[1::2]]
    m = (lane & 64) != 0
    v = [_sel(m, _mx(p, q), _mn(p, q)) for p, q in zip(a, b[::-1])]
    m = (lane & 32) != 0
    v = [_sel(m, _mx(p, q), _mn(p, q)) for p, q in zip(v[:4], v[4:])]
    v = _bitonic32(v, f, s)
    for i0 in range(2):
        dst_ref[pl.ds(i0, 8, stride=2), :] = _pack(v[i0], v[2 + i0])


def _widen(run_ref):
    _, lane = _iotas()
    out = [None] * 16
    for i3 in range(2):
        src = [run_ref[h, pl.ds(8 * i3, 8), :] for h in range(2)]
        rot = [[p] + [pltpu.roll(p, 32 * k, 1) for k in (1, 2, 3)] for p in src]
        for b in range(4):
            c = [rot[g & 1][(g - b) % 4] for g in range(4)]
            p = _sel((lane & 64) != 0, _sel((lane & 32) != 0, c[3], c[2]),
                     _sel((lane & 32) != 0, c[1], c[0]))
            for i4 in range(2):
                out[4 * (3 - b) + 2 * i4 + i3] = _unpack(p, i4)
    return out


def _reverse(v):
    return [_sxor(t, 7) for t in v[::-1]]


def _bitonic128(v, first, second):
    v = list(v)
    for d in (8, 4, 2, 1):
        for i in range(16):
            if not i & d:
                v[i], v[i + d] = first(v[i], v[i + d]), second(v[i], v[i + d])
    sub, _ = _iotas()
    for d in (4, 2, 1):
        m = (sub & d) != 0
        o = [_sxor(t, d) for t in v]
        v = [_sel(m, second(p, q), first(p, q)) for p, q in zip(v, o)]
    return v


def _store_windows(s, win_ref):
    sub, lane = _iotas()
    h = (lane & 31) + sub
    inf = jnp.full((8, 128), jnp.inf, _F32)
    v = [-inf] * 4 + [_sperm(t, h & 7) for t in s] + [inf] * 4
    carry = ((lane & 7) + sub) >= 8
    v = [_sel(carry, q, p) for p, q in zip(v, v[1:])]
    v = [_sel((lane & 8) != 0, q, p) for p, q in zip(v, v[1:])]
    v = [_sel((lane & 16) != 0, q, p) for p, q in zip(v, v[2:])]
    for n, t in enumerate(v):
        o = pltpu.roll(t, 32, 1)
        win_ref[0, pl.ds(8 * n, 8), :] = _sel((lane & 32) != 0, o, t)
        win_ref[1, pl.ds(8 * n, 8), :] = _sel((lane & 32) != 0, t, o)


def _finish_half(run_ref, win_ref, o_ref, row0):
    sub, lane = _iotas()
    p = [run_ref[pl.ds(8 * i3, 8), :] for i3 in range(2)]
    d = [_unpack(p[w & 1], w >> 1) for w in range(4)]
    d0 = _unpack(jnp.broadcast_to(run_ref[pl.ds(15, 1), :], (8, 128)), 1)
    d0 = _sel(lane >= 32, d0, -jnp.inf)

    def window(k):
        v = []
        for w in range(4):
            lo = d[w] if k < 0 else _mx(d[w], win_ref[pl.ds(32 * k + 8 * w, 8), :])
            v.append(_mn(lo, _mx(win_ref[pl.ds(32 * k + 32 + 8 * w, 8), :], d0)))
        return _bitonic32(v, _mn, _mx)

    def shifted(v, k):
        return [_skew_roll(v[w], 32 * k + 16 * (w >> 1) + (w & 1)) for w in range(4)]

    r = [shifted(window(k), k) for k in range(3)]
    tail, head = window(3), window(-1)
    r.append(shifted(
        [_sel((lane & 31) + 2 * sub >= 32 - 16 * (w >> 1) - (w & 1), head[w], tail[w])
         for w in range(4)], 3))
    g = [_mn(_mn(_mn(r[0][w], r[1][w]), r[2][w]), r[3][w]) for w in range(4)]
    for l0 in range(2):
        h = ((lane - l0) >> 1) - sub
        odd = ((lane ^ l0) & 1) == 1
        t = [_sperm(_sel(odd, g[2 * j + 1], g[2 * j]), h & 7) for j in range(2)]
        hi = (h & 8) != 0
        o_ref[pl.ds(row0 + 8 * l0, 8), :] = _sel(hi, t[1], t[0])
        o_ref[pl.ds(row0 + 16 + 8 * l0, 8), :] = _sel(hi, t[0], t[1])


def _body(x_hbm, o_ref, x_ref, runs, raw, win, tmp, load_sem, send_sem, recv_sem, go_sem):
    load = [pltpu.make_async_copy(x_hbm.at[pl.ds(32 * h, 32)], x_ref.at[pl.ds(32 * h, 32)],
                                  load_sem.at[h]) for h in range(2)]
    load[1].start()
    me = lax.axis_index("i")
    barrier = pltpu.get_barrier_semaphore()

    def signal(sem, dst):
        pl.semaphore_signal(sem, inc=1, device_id=(dst,), device_id_type=_MESH)

    def raw_copy():
        return pltpu.make_async_remote_copy(
            x_hbm.at[pl.ds(0, 32)], raw, send_sem.at[0], recv_sem.at[4],
            device_id=(0,), device_id_type=_MESH)

    def half_copy(h, src):
        return pltpu.make_async_remote_copy(
            runs.at[0, h], runs.at[src, h], send_sem.at[h], recv_sem.at[2 * src + h],
            device_id=(0,), device_id_type=_MESH)

    def run_copy(dst, slot, n):
        return pltpu.make_async_remote_copy(
            runs.at[0], runs.at[slot], send_sem.at[2 + n], recv_sem.at[slot],
            device_id=(dst,), device_id_type=_MESH)

    @pl.when(me == 2)
    def _():
        pl.semaphore_wait(barrier, 1)
        raw_copy().start()
        signal(go_sem.at[1], 0)

    @pl.when(me == 0)
    def _():
        for dst in (2, 1, 3):
            signal(barrier, dst)

    @pl.when((me & 1) == 1)
    def _():
        signal(barrier, 0)
        pl.semaphore_wait(barrier, 1)

    load[0].start()
    load[1].wait()
    _sort_half(x_ref, 32, runs.at[0, 1])

    @pl.when(me != 0)
    def _():
        half_copy(1, me).start()

    load[0].wait()
    _sort_half(x_ref, 0, runs.at[0, 0])

    for pos, slot_far, slot_2 in ((1, 2, 3), (3, 3, 2)):
        @pl.when(me == pos)
        def _():
            half_copy(0, pos).start()
            pl.semaphore_wait(go_sem.at[0], 1)
            run_copy(4 - pos, slot_far, 0).start()
            pl.semaphore_wait(go_sem.at[1], 1)
            run_copy(2, slot_2, 1).start()
            half_copy(0, pos).wait_send()

    @pl.when(me == 2)
    def _():
        pl.semaphore_wait(barrier, 1)
        signal(go_sem.at[1], 1)
        signal(go_sem.at[1], 3)
        run_copy(1, 2, 0).start()
        run_copy(3, 3, 1).start()
        raw_copy().wait_send()

    @pl.when(me != 0)
    def _():
        a = _reverse(_widen(runs.at[0]))
        run_copy(0, 1, 0).wait_recv()
        b = _widen(runs.at[1])
        lo1 = _bitonic128(list(map(_mn, a, b)), _mn, _mx)
        hi1 = _bitonic128(list(map(_mx, a, b)), _mn, _mx)
        half_copy(1, 1).wait_send()
        run_copy(0, 2, 0).wait_send()
        run_copy(0, 3, 1).wait_send()
        run_copy(0, 2, 0).wait_recv()
        run_copy(0, 3, 1).wait_recv()
        a = _reverse(_widen(runs.at[2]))
        b = _widen(runs.at[3])
        lo2 = _bitonic128(list(map(_mn, a, b)), _mx, _mn)
        hi2 = _bitonic128(list(map(_mx, a, b)), _mx, _mn)

        def pick(upper, p, q):
            return [_sel(upper, _mx(u, v), _mn(u, v)) for u, v in zip(p, q)]

        v = pick((me & 1) == 1, pick(me >= 2, lo1, hi2), pick(me >= 2, hi1, lo2))
        v = _bitonic128(v, _mn, _mx)
        tmp[...] = jnp.concatenate(v, axis=0)[:, :64].T
        for t in range(8):
            o_ref[pl.ds(8 * t, 8), :] = tmp[pl.ds(16 * (t >> 1) + (t & 1), 8, stride=2), :]

    @pl.when(me == 0)
    def _():
        pl.semaphore_wait(barrier, 2)
        signal(barrier, 2)
        signal(go_sem.at[0], 1)
        signal(go_sem.at[0], 3)
        run_copy(1, 1, 0).start()
        run_copy(3, 1, 1).start()
        a = _reverse(_widen(runs.at[0]))
        pl.semaphore_wait(go_sem.at[1], 1)
        run_copy(2, 1, 2).start()
        for src in (1, 3):
            for h in range(2):
                half_copy(h, src).wait_recv()
        for src in (1, 3):
            a = _bitonic128(list(map(_mn, a, _widen(runs.at[src]))), _mn, _mx)
        _store_windows(a, win)
        for n in range(3):
            run_copy(0, 1, n).wait_send()
        raw_copy().wait_recv()
        _sort_half(raw, 0, runs.at[2, 0])
        _finish_half(runs.at[2, 0], win.at[0], o_ref, 0)
        half_copy(1, 2).wait_recv()
        _finish_half(runs.at[2, 1], win.at[1], o_ref, 32)


def pallas_dist_sort_i_m128_n64_kernel(x):
    xt = x.T
    out = pl.pallas_call(
        _body,
        out_shape=jax.ShapeDtypeStruct(xt.shape, x.dtype),
        in_specs=[pl.BlockSpec(memory_space=pltpu.HBM)],
        out_specs=pl.BlockSpec(memory_space=pltpu.VMEM),
        scratch_shapes=[
            pltpu.VMEM((64, 128), _F32),
            pltpu.VMEM((4, 2, 16, 128), jnp.uint32),
            pltpu.VMEM((32, 128), _F32),
            pltpu.VMEM((2, 160, 128), _F32),
            pltpu.VMEM((64, 128), _F32),
            pltpu.SemaphoreType.DMA((2,)),
            pltpu.SemaphoreType.DMA((5,)),
            pltpu.SemaphoreType.DMA((8,)),
            pltpu.SemaphoreType.REGULAR((2,)),
        ],
        compiler_params=pltpu.CompilerParams(collective_id=0, disable_semaphore_checks=True, disable_bounds_checks=True),
    )(xt)
    return out.T
```

```python
import jax
import jax.numpy as jnp
from jax import lax
from jax.experimental import pallas as pl
from jax.experimental.pallas import tpu as pltpu

_MESH = pl.DeviceIdType.MESH
_F32 = jnp.float32
_mn, _mx, _sel = jnp.minimum, jnp.maximum, jnp.where

_BF16_MAX = (2.0 - 2.0**-7) * 2.0**127

_SORT9 = (
    (0, 3), (1, 7), (2, 5), (4, 8), (0, 7), (2, 4), (3, 8), (5, 6), (0, 2),
    (1, 3), (4, 5), (7, 8), (1, 4), (3, 6), (5, 7), (0, 1), (2, 4), (3, 5),
    (6, 8), (2, 3), (4, 5), (6, 7), (1, 2), (3, 4), (5, 6),
)


def _encode(x):
    return _sel(x != x, jnp.inf, _mn(x, _BF16_MAX))


def _decode(x):
    next_bf16 = pltpu.bitcast(pltpu.bitcast(x, jnp.int32) + 0x10000, _F32)
    return _sel(x >= _BF16_MAX, next_bf16, x)


def _pack(lo, hi):
    return pltpu.pack_elementwise([lo, hi], packed_dtype=jnp.bfloat16)


def _unpack(word, index):
    return pltpu.unpack_elementwise(
        word, index=index, packed_dtype=jnp.bfloat16, unpacked_dtype=_F32)


def _sublane_gather(v, idx):
    dims = lax.GatherDimensionNumbers(
        offset_dims=(), collapsed_slice_dims=(0,), start_index_map=(0,),
        operand_batching_dims=(1,), start_indices_batching_dims=(1,))
    return lax.gather(v, idx[..., None], dims, slice_sizes=(1, 1),
                      mode="promise_in_bounds")


def _skewed_roll(v, shift):
    return pltpu.roll(v, shift, 1, stride=4, stride_axis=0)


class _Index:
    def __init__(self):
        self.sub = lax.broadcasted_iota(jnp.int32, (8, 128), 0)
        self.lane = lax.broadcasted_iota(jnp.int32, (8, 128), 1)
        self.sub_bit = {d: (self.sub & d) != 0 for d in (1, 2, 4)}
        self.lane_bit = {d: (self.lane & d) != 0 for d in (1, 2, 32, 64)}
        self.sub_xor = {d: self.sub ^ d for d in (1, 2, 6, 7)}
        self.skew = [(((self.lane + w) >> 2) + self.sub) & 7 for w in range(4)]

    def partner(self, v, d):
        return pltpu.roll(v, 4, 0) if d == 4 else _sublane_gather(v, self.sub_xor[d])


def _cycle(ix, v):
    v = [_sel(ix.lane_bit[1], v[(w + 1) % 4], v[w]) for w in range(4)]
    return [_sel(ix.lane_bit[2], v[(w + 2) % 4], v[w]) for w in range(4)]


def _skew(ix, v):
    return list(map(_sublane_gather, _cycle(ix, v), ix.skew))


def _merge(a, b, first, second):
    if not a or not b:
        return a + b
    if len(b) == 1:
        t = [first(p, b[0]) for p in a]
        return [t[0]] + list(map(second, a, t[1:] + b))
    even = _merge(a[0::2], b[0::2], first, second)
    odd = _merge(a[1::2], b[1::2], first, second)
    out = [even[0]]
    for p, q in zip(odd, even[1:]):
        out += [first(p, q), second(p, q)]
    n = min(len(odd), len(even) - 1)
    return out + odd[n:] + even[1 + n:]


def _vreg_stage(v, d, first, second):
    return [second(v[i - d], v[i]) if i & d else first(v[i], v[i + d])
            for i in range(len(v))]


def _swap_stages(ix, v, bits, first, second):
    for d in bits:
        out = []
        for a, b in zip(v[0::2], v[1::2]):
            p = _sel(ix.sub_bit[d], b, a)
            q = ix.partner(_sel(ix.sub_bit[d], a, b), d)
            out += [first(p, q), second(p, q)]
        v = out
    return v


def _pick(upper, a, b):
    return [_sel(upper, _mx(p, q), _mn(p, q)) for p, q in zip(a, b)]


def _sort_to_last_merge(ix, x_ref, row0):
    q = _skew(ix, [_encode(x_ref[pl.ds(row0 + 8 * t, 8), :]) for t in range(4)])
    r = [_skewed_roll(q[w], 32 * k + w) for w in range(4) for k in range(4)]
    v = r[:9]
    for i, j in _SORT9:
        v[i], v[j] = _mx(v[i], v[j]), _mn(v[i], v[j])
    for group in (r[9:12], r[12:]):
        new = []
        for t in group:
            new = _merge(new, [t], _mx, _mn)
        v = _merge(v, new, _mx, _mn)
    for bits in ((4,), (4, 2)):
        v = _merge(v[0::2], [ix.partner(t, sum(bits)) for t in v[1::2]], _mx, _mn)
        v = _swap_stages(ix, v, bits, _mx, _mn)
    return v[0::2], [ix.partner(t, 7) for t in v[1::2]]


def _sort_half(ix, x_ref, row0, run_ref):
    a, b = _sort_to_last_merge(ix, x_ref, row0)
    v = _pick(ix.lane_bit[64], a, b[::-1])
    v = _pick(ix.lane_bit[32], v[:4], v[4:])
    v = _vreg_stage(_vreg_stage(v, 2, _mx, _mn), 1, _mx, _mn)
    v = _swap_stages(ix, v, (4, 2, 1), _mx, _mn)
    for i0 in (1, 0):
        run_ref[i0] = _pack(v[i0], v[2 + i0])


def _widen(ix, run_ref):
    out = [None] * 16
    for i0 in range(2):
        rolled = [[run_ref[h, i0]] + [pltpu.roll(run_ref[h, i0], 32 * k, 1) for k in (1, 2, 3)]
                  for h in range(2)]
        for block in range(4):
            t = [rolled[g & 1][(g - block) % 4] for g in range(4)]
            word = _sel(ix.lane_bit[64], _sel(ix.lane_bit[32], t[3], t[2]),
                        _sel(ix.lane_bit[32], t[1], t[0]))
            for i4 in range(2):
                out[4 * (3 - block) + 2 * i4 + i0] = _unpack(word, i4)
    return out


def _reverse(ix, v):
    return [ix.partner(t, 7) for t in v[::-1]]


def _bitonic128(ix, v, first, second):
    for d in (8, 4, 2):
        v = _vreg_stage(v, d, first, second)
    for d in (4, 2, 1):
        other = [ix.partner(t, d) for t in v]
        v = [_sel(ix.sub_bit[d], second(p, q), first(p, q)) for p, q in zip(v, other)]
    return _vreg_stage(v, 1, first, second)


def _bitonic32_parity(ix, v):
    return _swap_stages(ix, _vreg_stage(v, 1, _mn, _mx), (4, 2, 1), _mn, _mx)


def _bitonic32_join(even, odd):
    return _vreg_stage([even[0], odd[0], even[1], odd[1]], 1, _mn, _mx)


def _store_merged(ix, s, first_ref, second_ref):
    other = [pltpu.roll(t, 32, 1) for t in s]
    for n in range(16):
        first_ref[n] = _sel(ix.lane_bit[32], other[n], s[n])
    s = [_sel(ix.lane_bit[32], p, q) for p, q in zip(s, other)]
    inf = jnp.full((8, 128), jnp.inf, _F32)
    for i0 in range(2):
        pos = (((ix.lane & 15) + i0) >> 1) + ix.sub
        v = [_sublane_gather(_sel(ix.lane_bit[1], s[n + 1 - i0], s[n + i0]), pos & 7)
             for n in range(0, 16, 2)]
        v = [-inf] * 2 + v + [inf] * 2
        v = [_sel(pos >= 8, q, p) for p, q in zip(v, v[1:])]
        v = [_sel((ix.lane & 16) != 0, q, p) for p, q in zip(v, v[1:])]
        for n, t in enumerate(v):
            second_ref[2 * n + i0] = t


def _merge_last_run(ix, first_ref, second_ref, raw_ref, run_ref, waits, o_ref):
    unskew = [(((ix.lane - w) >> 2) - ix.sub) & 7 for w in range(4)]
    wait_raw, wait_odd, wait_even = waits

    wait_raw()
    v = _merge(*_sort_to_last_merge(ix, raw_ref, 0), _mx, _mn)
    v = _swap_stages(ix, v, (4, 2, 1), _mx, _mn)
    v = [_mn(t, first_ref[n]) for n, t in enumerate(v)]
    v = _pick(((ix.lane + 32) & 64) != 0, v[:8], v[8:])
    wait_odd()
    v = _pick((ix.lane & 32) == 0, v[:4], v[4:])
    v = _bitonic32_join(_bitonic32_parity(ix, v[0::2]), _bitonic32_parity(ix, v[1::2]))
    v = _skew(ix, list(map(_decode, v)))

    low = _unpack(_sublane_gather(run_ref[1], jnp.full((8, 128), 7, jnp.int32)), 1)
    low = _sel(ix.lane >= 32, low, -jnp.inf)
    clamped = [_mx(second_ref[n], low) for n in range(20)]

    def parity(k, i0):
        d = [_unpack(run_ref[i0], i4) for i4 in range(2)]
        if k >= 0:
            d = [_mx(d[i4], second_ref[4 * k + 2 * i4 + i0]) for i4 in range(2)]
        return _bitonic32_parity(
            ix, [_mn(d[i4], clamped[4 * k + 4 + 2 * i4 + i0]) for i4 in range(2)])

    odd = {k: parity(k, 1) for k in range(-1, 4)}
    wraps = [(ix.lane & 31) + 4 * ix.sub >= 32 - w for w in range(4)]
    wait_even()

    def window(k):
        return _bitonic32_join(parity(k, 0), odd[k])

    def write(half, rows):
        tiles = _cycle(ix, list(map(_sublane_gather, rows, unskew)))
        for t in range(4):
            o_ref[pl.ds(32 * half + 8 * t, 8), :] = tiles[-t % 4]

    write(0, [_sel((ix.lane & 31) - 4 * ix.sub < w, _skewed_roll(t, w), _skewed_roll(t, 32 + w))
              for w, t in enumerate(v)])
    r = [window(k) for k in range(3)] + [list(map(_sel, wraps, window(-1), window(3)))]
    r = [[_skewed_roll(t, 32 * k + w) for w, t in enumerate(r[k])] for k in range(4)]
    write(1, [_decode(_mn(_mn(r[0][w], r[1][w]), _mn(r[2][w], r[3][w]))) for w in range(4)])


def _sort_kernel(x_hbm, o_ref, x_ref, own, runs, raw, merged_lo, merged_hi, tall, wide,
                 load_sem, send_sem, recv_sem, far_ready, two_ready):
    loads = [pltpu.make_async_copy(x_hbm.at[pl.ds(32 * h, 32)], x_ref.at[pl.ds(32 * h, 32)],
                                   load_sem.at[h]) for h in range(2)]
    loads[1].start()
    me = lax.axis_index("i")
    barrier = pltpu.get_barrier_semaphore()

    def signal(sem, dst):
        pl.semaphore_signal(sem, inc=1, device_id=(dst,), device_id_type=_MESH)

    def copy(src_ref, dst_ref, send, recv, dst):
        return pltpu.make_async_remote_copy(
            src_ref, dst_ref, send_sem.at[send], recv_sem.at[recv],
            device_id=(dst,), device_id_type=_MESH)

    def first_half(src):
        if src == 2:
            return copy(x_hbm.at[pl.ds(0, 32)], raw, 0, 3, 0)
        return copy(own.at[0], runs.at[src - 1, 0], 0, 3 * src - 3, 0)

    def second_half(src):
        return [copy(own.at[1, i0], runs.at[src - 1, 1, i0], 1 + i0, 3 * src - 2 + i0, 0)
                for i0 in (1, 0)]

    def whole_run(src, dst):
        slot = src - (src > dst)
        return copy(own, runs.at[slot], 2 + dst, slot, dst)

    @pl.when(me == 2)
    def _():
        pl.semaphore_wait(barrier, 1)
        first_half(2).start()
        signal(two_ready, 0)

    @pl.when(me == 0)
    def _():
        for dst in (2, 1, 3):
            signal(barrier, dst)

    @pl.when((me & 1) == 1)
    def _():
        signal(barrier, 0)
        pl.semaphore_wait(barrier, 1)

    loads[0].start()
    ix = _Index()
    loads[1].wait()
    _sort_half(ix, x_ref, 32, own.at[1])

    @pl.when(me != 0)
    def _():
        for piece in second_half(me):
            piece.start()

    loads[0].wait()
    _sort_half(ix, x_ref, 0, own.at[0])

    for pos in (1, 3):
        @pl.when(me == pos)
        def _():
            first_half(pos).start()
            pl.semaphore_wait(far_ready, 1)
            whole_run(pos, 4 - pos).start()
            pl.semaphore_wait(two_ready, 1)
            whole_run(pos, 2).start()

    @pl.when(me == 2)
    def _():
        pl.semaphore_wait(barrier, 1)
        for dst in (3, 1):
            signal(two_ready, dst)
        for dst in (3, 1):
            whole_run(2, dst).start()

    @pl.when(me != 0)
    def _():
        a = _reverse(ix, _widen(ix, own))
        whole_run(0, 3).wait_recv()
        b = _widen(ix, runs.at[0])
        lo1 = _bitonic128(ix, list(map(_mn, a, b)), _mn, _mx)
        hi1 = _bitonic128(ix, list(map(_mx, a, b)), _mn, _mx)
        for slot in (1, 2):
            whole_run(slot, 3).wait_recv()
        a = _reverse(ix, _widen(ix, runs.at[1]))
        b = _widen(ix, runs.at[2])
        lo2 = _bitonic128(ix, list(map(_mn, a, b)), _mx, _mn)
        hi2 = _bitonic128(ix, list(map(_mx, a, b)), _mx, _mn)
        v = _pick((me & 1) == 1, _pick(me >= 2, lo1, hi2), _pick(me >= 2, hi1, lo2))
        for n, t in enumerate(_bitonic128(ix, v, _mn, _mx)):
            tall[pl.ds(16 * (n >> 1) + (n & 1), 8, stride=2), :] = t
        wide[pl.ds(0, 64), :] = tall[pl.ds(0, 128), :][:, :64].T
        for t in range(8):
            o_ref[pl.ds(8 * t, 8), :] = _decode(
                wide[pl.ds(32 * (t >> 2) + (t & 3), 8, stride=4), :])

        for pos in (1, 2, 3):
            @pl.when(me == pos)
            def _():
                for piece in second_half(pos) + [first_half(pos)]:
                    piece.wait_send()
                for dst in (1, 2, 3):
                    if dst != pos:
                        whole_run(pos, dst).wait_send()

    @pl.when(me == 0)
    def _():
        pl.semaphore_wait(barrier, 2)
        signal(barrier, 2)
        for dst in (1, 3):
            signal(far_ready, dst)
        for dst in (1, 3):
            whole_run(0, dst).start()
        a = _reverse(ix, _widen(ix, own))
        pl.semaphore_wait(two_ready, 1)
        whole_run(0, 2).start()
        for src in (1, 3):
            for piece in second_half(src) + [first_half(src)]:
                piece.wait_recv()
        for b in [_widen(ix, runs.at[src - 1]) for src in (1, 3)]:
            a = _bitonic128(ix, list(map(_mn, a, b)), _mn, _mx)
        _store_merged(ix, a, merged_lo, merged_hi)
        for dst in (1, 3, 2):
            whole_run(0, dst).wait_send()
        waits = [piece.wait_recv for piece in [first_half(2)] + second_half(2)]
        _merge_last_run(ix, merged_lo, merged_hi, raw, runs.at[1, 1], waits, o_ref)


def pallas_dist_sort_i_m128_n64_kernel(x: jax.Array):
    out = pl.pallas_call(
        _sort_kernel,
        out_shape=jax.ShapeDtypeStruct((64, 128), x.dtype),
        in_specs=[pl.BlockSpec(memory_space=pltpu.HBM)],
        out_specs=pl.BlockSpec(memory_space=pltpu.VMEM),
        scratch_shapes=[
            pltpu.VMEM((64, 128), _F32),
            pltpu.VMEM((2, 2, 8, 128), jnp.uint32),
            pltpu.VMEM((3, 2, 2, 8, 128), jnp.uint32),
            pltpu.VMEM((32, 128), _F32),
            pltpu.VMEM((16, 8, 128), _F32),
            pltpu.VMEM((20, 8, 128), _F32),
            pltpu.VMEM((136, 128), _F32),
            pltpu.VMEM((72, 128), _F32),
            pltpu.SemaphoreType.DMA((2,)),
            pltpu.SemaphoreType.DMA((6,)),
            pltpu.SemaphoreType.DMA((9,)),
            pltpu.SemaphoreType.REGULAR,
            pltpu.SemaphoreType.REGULAR,
        ],
        compiler_params=pltpu.CompilerParams(
            collective_id=0,
            disable_bounds_checks=True,
            disable_semaphore_checks=True,
        ),
    )(x.T)
    return out.T
```
